```python
import numpy as np

kernel_name = "dist_mlpseq_tp1d_rep_rep_b128_d128_h256"

def setup_inputs():
    x = np.random.randn(128, 128).astype(np.float32)
    Win0 = np.random.randn(128, 1024).astype(np.float32)
    Wout0 = np.random.randn(1024, 128).astype(np.float32)
    Win1 = np.random.randn(128, 1024).astype(np.float32)
    Wout1 = np.random.randn(1024, 128).astype(np.float32)
    Win2 = np.random.randn(128, 1024).astype(np.float32)
    Wout2 = np.random.randn(1024, 128).astype(np.float32)
    return {"x": x, "Win0": Win0, "Wout0": Wout0, "Win1": Win1, "Wout1": Wout1, "Win2": Win2, "Wout2": Wout2}

def reference(x, Win0, Win1, Win2, Wout0, Wout1, Wout2):
    h = x @ Win0
    h = np.maximum(h, 0.0)
    x = h @ Wout0
    h = x @ Win1
    h = np.maximum(h, 0.0)
    x = h @ Wout1
    h = x @ Win2
    h = np.maximum(h, 0.0)
    x = h @ Wout2
    return x
```

```python
import jax
import jax.numpy as jnp
from jax import lax
from jax.experimental import pallas as pl
from jax.experimental.pallas import tpu as pltpu

N_LAYERS = 3
N_CHUNKS = 4

_ORDER = {
    (0, 0): "|g0 x0 y0 g1 x1||y1 g2 y2 x2 g3 y3 x3",
    (0, 1): "g0 y0|g1 y1 x0|g2 y2|g3 x1 x3 x2 y3",
    (0, 2): "x0|g0 x1|g2 y0 y1 g1|g3 x2 y2 y3 x3",
    (3, 0): "|x0 g0 g1 x1|y1 g2|x3 y2 g3 y3 x2 y0",
    (3, 1): "g0 y0|g1 y1|g2 x0 y2|g3 y3 x3 x2 x1",
    (3, 2): "g0 x0|g1 x1|x2 y0|y2 x3 g2 y1 y3 g3",
    (1, 0): "|y1 g0 g1 y0|y2 x2 x1|g2 x0 x3 y3 g3",
    (1, 1): "g0 x0|x1 y0|g1 x2 y1|g2 y2 g3 y3 x3",
    (1, 2): "y0|y1|x1 g1 x0 y2|y3 g3 g0 g2 x2 x3",
    (2, 0): "g0|g1 y0 x0|g2 y1 x1|g3 x2 x3 y2 y3",
    (2, 1): "g0 x0|y0 y1 g1 x1|x2 y2 g2|g3 y3 x3",
    (2, 2): "g0|g1|g2|g3 y3 x2 y2 y0 x3 x1 x0 y1",
}
_BRANCH_ORDER = ((2, 0, 1, 3), (0, 2, 1, 3), (2, 0, 1, 3))
_SLOT_OF = {"g": 0, "x": 1, "y": 2}


def _slots(dev, layer):
    return [
        tuple((m[0], int(m[1:])) for m in s.split())
        for s in _ORDER[(dev, layer)].split("|")
    ]


def _any_of(my, devs):
    cond = my == devs[0]
    for d in devs[1:]:
        cond = jnp.logical_or(cond, my == d)
    return cond


def pallas_dist_mlpseq_tp1d_rep_rep_b128_d128_h256_kernel(
    x: jax.Array,
    Win0: jax.Array,
    Wout0: jax.Array,
    Win1: jax.Array,
    Wout1: jax.Array,
    Win2: jax.Array,
    Wout2: jax.Array,
):
    B, D = x.shape
    H = Win0.shape[1]
    L, NC = N_LAYERS, N_CHUNKS
    R = B // NC
    bf16, f32 = jnp.bfloat16, jnp.float32

    def body(x_hbm, wi0, wo0, wi1, wo1, wi2, wo2, out_ref,
             xv, wiv, wov, wib, wob, sendb, recvb, sent_dummy,
             in_sems, send_sems, recv_sems):
        my = lax.axis_index("i")
        peers = {"g": my ^ 2, "x": 3 - my, "y": my ^ 1}

        def rows(c):
            return pl.ds(c * R, R)

        wis, wos = (wi0, wi1, wi2), (wo0, wo1, wo2)
        cwi = [pltpu.make_async_copy(wis[l], wiv.at[l], in_sems.at[2 + 2 * l])
               for l in range(L)]
        cwo = [pltpu.make_async_copy(wos[l], wov.at[l], in_sems.at[3 + 2 * l])
               for l in range(L)]
        cx0 = pltpu.make_async_copy(
            x_hbm.at[pl.ds(0, R)], xv.at[pl.ds(0, R)], in_sems.at[0])
        cx1 = pltpu.make_async_copy(
            x_hbm.at[pl.ds(R, B - R)], xv.at[pl.ds(R, B - R)], in_sems.at[1])
        cx0.start()
        cwi[0].start()
        cwo[0].start()
        cx1.start()
        barrier = pltpu.get_barrier_semaphore()
        for p in peers.values():
            pl.semaphore_signal(barrier, 1, device_id=(p,),
                                device_id_type=pl.DeviceIdType.MESH)

        def rcopy(l, c, kind):
            return pltpu.make_async_remote_copy(
                src_ref=sendb.at[l, rows(c)],
                dst_ref=recvb.at[l, c, _SLOT_OF[kind]],
                send_sem=send_sems.at[l],
                recv_sem=recv_sems.at[l, c],
                device_id=(peers[kind],),
                device_id_type=pl.DeviceIdType.MESH)

        def wait_recv(l, c):
            r = recvb.at[l, c]
            pltpu.make_async_copy(r, r, recv_sems.at[l, c]).wait()

        def wait_sends(l):
            pltpu.make_async_copy(sent_dummy, sent_dummy, send_sems.at[l]).wait()

        def send_slot(l, c):
            groups = {}
            for dev in _BRANCH_ORDER[l]:
                groups.setdefault(_slots(dev, l)[c], []).append(dev)
            for msgs, devs in groups.items():
                if not msgs:
                    continue

                @pl.when(_any_of(my, devs))
                def _():
                    for kind, k in msgs:
                        rcopy(l, k, kind).start()

        cx0.wait()
        cwi[0].wait()
        wi0b = wiv[0].astype(bf16)
        wib[0] = wi0b
        h00 = jnp.dot(xv[rows(0), :].astype(bf16), wi0b,
                      preferred_element_type=f32)
        h00 = jnp.maximum(h00, 0.0).astype(bf16)

        @pl.when(my >= 0)
        def _():
            cwo[0].wait()
            for l in range(1, L):
                cwi[l].start()
                cwo[l].start()

        wo0b = wov[0].astype(bf16)
        wob[0] = wo0b

        first_slot = {
            dev: min(i for i, s in enumerate(_slots(dev, 0)) if s)
            for dev in range(4)
        }

        own = [None] * NC
        for l in range(L):
            for c in range(NC):
                if l > 0:
                    wait_recv(l - 1, c)
                elif c == 1:
                    cx1.wait()
                if l == 0 and c == 0:
                    p = jnp.dot(h00, wo0b, preferred_element_type=f32)
                else:
                    if l > 0:
                        acc = own[c]
                        for s in range(3):
                            acc = acc + recvb[l - 1, c, s].astype(f32)
                        xs = acc.astype(bf16)
                    else:
                        xs = xv[rows(c), :].astype(bf16)
                    h = jnp.dot(xs, wib[l], preferred_element_type=f32)
                    h = jnp.maximum(h, 0.0).astype(bf16)
                    p = jnp.dot(h, wob[l], preferred_element_type=f32)
                own[c] = p
                sendb[l, rows(c), :] = p.astype(bf16)
                if l == 0:
                    devs = [d for d in range(4) if first_slot[d] == c]
                    if devs:
                        @pl.when(_any_of(my, devs))
                        def _():
                            pl.semaphore_wait(barrier, 3)
                send_slot(l, c)
            if l + 1 < L:
                cwi[l + 1].wait()
                wib[l + 1] = wiv[l + 1].astype(bf16)
                cwo[l + 1].wait()
                wob[l + 1] = wov[l + 1].astype(bf16)
                if l > 0:
                    wait_sends(l - 1)
        wait_sends(L - 2)
        for c in range(NC):
            wait_recv(L - 1, c)
            acc = own[c]
            for s in range(3):
                acc = acc + recvb[L - 1, c, s].astype(f32)
            out_ref[rows(c), :] = acc
        wait_sends(L - 1)

    return pl.pallas_call(
        body,
        out_shape=jax.ShapeDtypeStruct((B, D), f32),
        in_specs=[pl.BlockSpec(memory_space=pl.ANY)] * 7,
        out_specs=pl.BlockSpec(memory_space=pltpu.VMEM),
        scratch_shapes=[
            pltpu.VMEM((B, D), f32),
            pltpu.VMEM((L, D, H), f32),
            pltpu.VMEM((L, H, D), f32),
            pltpu.VMEM((L, D, H), bf16),
            pltpu.VMEM((L, H, D), bf16),
            pltpu.VMEM((L, B, D), bf16),
            pltpu.VMEM((L, NC, 3, R, D), bf16),
            pltpu.VMEM((3, B, D), bf16),
            pltpu.SemaphoreType.DMA((2 + 2 * L,)),
            pltpu.SemaphoreType.DMA((L,)),
            pltpu.SemaphoreType.DMA((L, NC)),
        ],
        compiler_params=pltpu.CompilerParams(
            collective_id=0,
            disable_semaphore_checks=True,
            disable_bounds_checks=True,
        ),
    )(x, Win0, Wout0, Win1, Wout1, Win2, Wout2)
```

```python
import jax
import jax.numpy as jnp
from jax import lax
from jax.experimental import pallas as pl
from jax.experimental.pallas import tpu as pltpu

N_LAYERS = 3
N_CHUNKS = 4

_ORDER = {
    (0, 0): "|g0 x0 y0 g1 x1||y1 g2 y2 x2 g3 y3 x3",
    (0, 1): "g0 y0|g1 y1 x0|g2 y2|g3 x1 x3 x2 y3",
    (0, 2): "x0|g0 x1|g2 y0 y1 g1|g3 x2 y2 y3 x3",
    (3, 0): "|x0 g0 g1 x1|y1 g2|x3 y2 g3 y3 x2 y0",
    (3, 1): "g0 y0|g1 y1|g2 x0 y2|g3 y3 x3 x2 x1",
    (3, 2): "g0 x0|g1 x1|x2 y0|y2 x3 g2 y1 y3 g3",
    (1, 0): "|y1 g0 g1 y0|y2 x2 x1|g2 x0 x3 y3 g3",
    (1, 1): "g0 x0|x1 y0|g1 x2 y1|g2 y2 g3 y3 x3",
    (1, 2): "y0|y1|x1 g1 x0 y2|y3 g3 g0 g2 x2 x3",
    (2, 0): "g0|g1 y0 x0|g2 y1 x1|g3 x2 x3 y2 y3",
    (2, 1): "g0 x0|y0 y1 g1 x1|x2 y2 g2|g3 y3 x3",
    (2, 2): "g0|g1|g2|g3 y3 x2 y2 y0 x3 x1 x0 y1",
}
_BRANCH_ORDER = ((2, 0, 1, 3), (0, 2, 1, 3), (2, 0, 1, 3))
_SLOT_OF = {"g": 0, "x": 1, "y": 2}


def _slots(dev, layer):
    return [
        tuple((m[0], int(m[1:])) for m in s.split())
        for s in _ORDER[(dev, layer)].split("|")
    ]


def _any_of(my, devs):
    cond = my == devs[0]
    for d in devs[1:]:
        cond = jnp.logical_or(cond, my == d)
    return cond


def pallas_dist_mlpseq_tp1d_rep_rep_b128_d128_h256_kernel(
    x: jax.Array,
    Win0: jax.Array,
    Wout0: jax.Array,
    Win1: jax.Array,
    Wout1: jax.Array,
    Win2: jax.Array,
    Wout2: jax.Array,
):
    B, D = x.shape
    H = Win0.shape[1]
    L, NC = N_LAYERS, N_CHUNKS
    R = B // NC
    bf16, f32 = jnp.bfloat16, jnp.float32

    def body(x_hbm, wi0, wo0, wi1, wo1, wi2, wo2, out_ref,
             xv, wiv, wov, sendb, recvb, sent_dummy,
             in_sems, send_sems, recv_sems):
        my = lax.axis_index("i")
        peers = {"g": my ^ 2, "x": 3 - my, "y": my ^ 1}

        def rows(c):
            return pl.ds(c * R, R)

        wis, wos = (wi0, wi1, wi2), (wo0, wo1, wo2)
        cwi = [pltpu.make_async_copy(wis[l], wiv.at[l], in_sems.at[2 + 2 * l])
               for l in range(L)]
        cwo = [pltpu.make_async_copy(wos[l], wov.at[l], in_sems.at[3 + 2 * l])
               for l in range(L)]
        cx0 = pltpu.make_async_copy(
            x_hbm.at[pl.ds(0, R)], xv.at[pl.ds(0, R)], in_sems.at[0])
        cx1 = pltpu.make_async_copy(
            x_hbm.at[pl.ds(R, B - R)], xv.at[pl.ds(R, B - R)], in_sems.at[1])
        cx0.start()
        cwi[0].start()
        cwo[0].start()
        cx1.start()
        barrier = pltpu.get_barrier_semaphore()
        for p in peers.values():
            pl.semaphore_signal(barrier, 1, device_id=(p,),
                                device_id_type=pl.DeviceIdType.MESH)

        def rcopy(l, c, kind):
            return pltpu.make_async_remote_copy(
                src_ref=sendb.at[l, rows(c)],
                dst_ref=recvb.at[l, c, _SLOT_OF[kind]],
                send_sem=send_sems.at[l],
                recv_sem=recv_sems.at[l, c],
                device_id=(peers[kind],),
                device_id_type=pl.DeviceIdType.MESH)

        def wait_recv(l, c):
            r = recvb.at[l, c]
            pltpu.make_async_copy(r, r, recv_sems.at[l, c]).wait()

        def wait_sends(l):
            pltpu.make_async_copy(sent_dummy, sent_dummy, send_sems.at[l]).wait()

        def send_slot(l, c):
            groups = {}
            for dev in _BRANCH_ORDER[l]:
                groups.setdefault(_slots(dev, l)[c], []).append(dev)
            for msgs, devs in groups.items():
                if not msgs:
                    continue

                @pl.when(_any_of(my, devs))
                def _():
                    for kind, k in msgs:
                        rcopy(l, k, kind).start()

        cx0.wait()
        cwi[0].wait()
        h00 = jnp.dot(xv[rows(0), :].astype(bf16), wiv[0].astype(bf16),
                      preferred_element_type=f32)
        h00 = jnp.maximum(h00, 0.0).astype(bf16)

        @pl.when(my >= 0)
        def _():
            cwo[0].wait()

        for l in range(1, L):
            cwi[l].start()
            cwo[l].start()

        first_slot = {
            dev: min(i for i, s in enumerate(_slots(dev, 0)) if s)
            for dev in range(4)
        }

        own = [None] * NC
        for l in range(L):
            for c in range(NC):
                if l > 0:
                    wait_recv(l - 1, c)
                elif c == 1:
                    cx1.wait()
                if l == 0 and c == 0:
                    p = jnp.dot(h00, wov[0].astype(bf16), preferred_element_type=f32)
                else:
                    if l > 0:
                        acc = own[c]
                        for s in range(3):
                            acc = acc + recvb[l - 1, c, s].astype(f32)
                        xs = acc.astype(bf16)
                    else:
                        xs = xv[rows(c), :].astype(bf16)
                    h = jnp.dot(xs, wiv[l].astype(bf16), preferred_element_type=f32)
                    h = jnp.maximum(h, 0.0).astype(bf16)
                    p = jnp.dot(h, wov[l].astype(bf16), preferred_element_type=f32)
                own[c] = p
                sendb[l, rows(c), :] = p.astype(bf16)
                if l == 0:
                    devs = [d for d in range(4) if first_slot[d] == c]
                    if devs:
                        @pl.when(_any_of(my, devs))
                        def _():
                            pl.semaphore_wait(barrier, 3)
                send_slot(l, c)
            if l + 1 < L:
                cwi[l + 1].wait()
                cwo[l + 1].wait()
                if l > 0:
                    wait_sends(l - 1)
        wait_sends(L - 2)
        for c in range(NC):
            wait_recv(L - 1, c)
            acc = own[c]
            for s in range(3):
                acc = acc + recvb[L - 1, c, s].astype(f32)
            out_ref[rows(c), :] = acc
        wait_sends(L - 1)

    return pl.pallas_call(
        body,
        out_shape=jax.ShapeDtypeStruct((B, D), f32),
        in_specs=[pl.BlockSpec(memory_space=pl.ANY)] * 7,
        out_specs=pl.BlockSpec(memory_space=pltpu.VMEM),
        scratch_shapes=[
            pltpu.VMEM((B, D), f32),
            pltpu.VMEM((L, D, H), f32),
            pltpu.VMEM((L, H, D), f32),
            pltpu.VMEM((L, B, D), bf16),
            pltpu.VMEM((L, NC, 3, R, D), bf16),
            pltpu.VMEM((3, B, D), bf16),
            pltpu.SemaphoreType.DMA((2 + 2 * L,)),
            pltpu.SemaphoreType.DMA((L,)),
            pltpu.SemaphoreType.DMA((L, NC)),
        ],
        compiler_params=pltpu.CompilerParams(
            collective_id=0,
            disable_semaphore_checks=True,
            disable_bounds_checks=True,
        ),
    )(x, Win0, Wout0, Win1, Wout1, Win2, Wout2)
```
